```python
import numpy as np

kernel_name = "dist_sparse_attn_blocksparse_kvseq_b2_sq256_skv256_hq4_dh64"

def setup_inputs():
    x = np.random.randn(2, 256, 512).astype(np.float32)
    Wq = np.random.randn(512, 256).astype(np.float32) * 0.02
    K_ext = np.random.randn(2, 1024, 4, 64).astype(np.float32)
    V_ext = np.random.randn(2, 1024, 4, 64).astype(np.float32)
    Wo = np.random.randn(256, 512).astype(np.float32) * 0.02
    return {"x": x, "Wq": Wq, "K_ext": K_ext, "V_ext": V_ext, "Wo": Wo}

def reference(x, Wq, K_ext, V_ext, Wo):
    B, Sq, Skv, Hq, Dh = 2, 256, 1024, 4, 64
    Q = (x @ Wq).reshape(B, Sq, Hq, Dh)
    qb = (np.arange(Sq) // 64)[:, None]
    kb = (np.arange(Skv) // 64)[None, :]
    mask = (qb == kb) | (kb == 0) | ((qb + kb) % 3 == 0)
    scores = np.einsum('bihd,bjhd->bhij', Q, K_ext).astype(np.float32) * 0.125
    scores = np.where(mask[None, None, :, :], scores, -1e9)
    scores_max = scores.max(axis=-1, keepdims=True)
    w = np.exp(scores - scores_max)
    row_keep = mask.any(axis=1)
    w_sum = np.where(row_keep[None, None, :, None], w.sum(axis=-1, keepdims=True), 1.0)
    w = w / w_sum
    w = np.where(row_keep[None, None, :, None], w, 0.0)
    ctx = np.einsum('bhij,bjhd->bihd', w, V_ext).reshape(B, Sq, Hq * Dh)
    return ctx @ Wo
```

```python
import jax
import jax.numpy as jnp
from jax import lax
from jax.experimental import pallas as pl
from jax.experimental.pallas import tpu as pltpu

MESH = pl.DeviceIdType.MESH
F32 = jnp.float32
BF16 = jnp.bfloat16
U32 = jnp.uint32
QSCALE = 0.125 * 1.4426950408889634
NT = (((1,), (1,)), ((), ()))
NN = (((1,), (0,)), ((), ()))
KVS = ("K", "V", "K0", "K1", "V0", "V1")
CLS = (0, 1, 2, 0)
SSPLIT = 2
BRANCH_ORDER = (2, 3, 1, 0)


def own_blks(dev, qb):
    return tuple(j for j in range(4)
                 if qb == 4 * dev + j or 4 * dev + j == 0 or (qb + 4 * dev + j) % 3 == 0)


def pv_tiles(need):
    if set(need) == {0, 3}:
        return [(0, 3)]
    return [t for t in ((0, 1), (2, 3)) if set(need) & set(t)]


def dot(a, b, dims):
    return lax.dot_general(a, b, dims, preferred_element_type=F32)


def merge_weights(lses):
    mx = lses[0]
    for z in lses[1:]:
        mx = jnp.maximum(mx, z)
    es = [jnp.exp2(z - mx) for z in lses]
    tot = es[0]
    for e in es[1:]:
        tot = tot + e
    inv = 1.0 / tot
    return [e * inv for e in es], mx + jnp.log2(tot)


def build(plan):
    msgs = plan["msgs"]
    mig = {(m["src"], m["b"], m["q"], m["p"]): m["dst"] for m in msgs if m["set"] in ("K", "K0")}
    route = lambda m: tuple(m[k] for k in ("src", "dst", "b", "q", "p", "set"))
    quarters = {}
    for m in msgs:
        quarters.setdefault(route(m), []).extend(m["subs"] or range(4))
    row_of = lambda m, h: 8 + 8 * sorted(quarters[route(m)]).index(h)

    def rows_of(m):
        subs = m["subs"] or range(4)
        row, n = row_of(m, subs[0]), 8 * len(subs)
        return (7, n + 1) if row == 8 and not isinstance(m["set"], str) else (row, n)

    def number(keys, chip):
        cnt, out = [0] * 4, {}
        for key in keys:
            if key not in out:
                out[key] = cnt[chip(key)]
                cnt[chip(key)] += 1
        return out, max(cnt)

    sslot, n_sbuf = number([route(m) for m in msgs], lambda r: r[0])
    rslot, n_rbuf = number([route(m) for m in msgs], lambda r: r[1])
    rsem_of, lsem_of = {}, {}
    for dev, prog in plan["prog"].items():
        for n, op in enumerate(op for op in prog if op[0] == "rwait"):
            rsem_of.update({i: n for i in op[1]})
        for n, op in enumerate(op for op in prog if op[0] == "wait"):
            lsem_of.update({(dev, name): n for name in op[1]})
    n_recv, n_load = max(rsem_of.values()) + 1, max(lsem_of.values()) + 1
    kib = lambda n: {"wq": 256, "wo": 512, "x": 128}.get(n[0]) or (128 if n[3] is None else 64)
    d0sig = any(m["src"] == 0 and m["dst"] == 2 for m in msgs)

    def contrib(b, qb, p):
        return frozenset(d for d in range(4) if (d, b, CLS[qb], p) not in mig)

    def body(x_hbm, wq_hbm, k_hbm, v_hbm, wo_hbm, o_ref, xb, wqb, kb, vb, wob, sbuf, rbuf, size_ref,
             lsem, ssem, rsem, dsem, fsem):
        my = lax.axis_index("i")
        bar = pltpu.get_barrier_semaphore()

        def sig(sem, d):
            pl.semaphore_signal(sem, inc=1, device_id=(d,), device_id_type=MESH)

        def wait_rows(sem, n):
            ref = size_ref.at[pl.ds(0, n)]
            pltpu.make_async_copy(ref, ref, sem).wait()

        def run(dev):
            loads = plan["loads"][dev]
            got = {(m["b"], m["q"], m["p"], h): m for m in msgs
                   if m["dst"] == dev and m["set"] == "T" for h in m["subs"]}

            def rdma(i):
                m = msgs[i]
                subs = m["subs"] or range(4)
                row, n = rows_of(m)
                src = sbuf.at[pl.ds(40 * sslot[route(m)] + row, n)]
                via = got.get((m["b"], m["q"], m["p"], subs[0])) if m["set"] == "T" else None
                if via is not None and m["src"] == dev:
                    src = rbuf.at[rslot[route(via)], pl.ds(row_of(via, subs[0]), n)]
                return pltpu.make_async_remote_copy(
                    src, rbuf.at[rslot[route(m)], pl.ds(row, n)],
                    ssem, rsem.at[rsem_of[i]],
                    device_id=(m["dst"],), device_id_type=MESH)

            def load(n):
                sem = lsem.at[lsem_of[dev, n]]
                if n[0] == "wq":
                    c = pl.ds(128 * n[1], 128)
                    return pltpu.make_async_copy(wq_hbm.at[:, c], wqb.at[:, c], sem)
                if n[0] == "wo":
                    return pltpu.make_async_copy(wo_hbm, wob, sem)
                if n[0] == "x":
                    r = pl.ds(64 * n[2], 64)
                    return pltpu.make_async_copy(x_hbm.at[n[1], r], xb.at[n[1], r], sem)
                src, dst = (k_hbm, kb) if n[0] == "k" else (v_hbm, vb)
                r = pl.ds(128 * n[2], 128)
                c = pl.ds(0, 256) if n[3] is None else pl.ds(128 * n[3], 128)
                return pltpu.make_async_copy(src.at[n[1], r, c], dst.at[n[1], r, c], sem)

            for n in loads[:2]:
                load(n).start()
            if dev == 0:
                sig(bar, 1)
                sig(bar, 3)
            elif dev != 2:
                sig(bar, 0)
                pl.semaphore_wait(bar, 1)
                sig(bar, 2)
            for n in loads[2:]:
                load(n).start()
            n_fence = sum(1 for op in plan["prog"][dev] if op[0] == "fence")
            if n_fence:
                pl.semaphore_signal(fsem, inc=n_fence)

            stores = {}
            val = {}
            acc = {}
            lses = {}
            left = lax.broadcasted_iota(jnp.int32, (64, 128), 1) < 64
            zero = jnp.zeros((64, 128), F32)

            def guests(b, qb, p):
                return [s for (s, bb, c, pp), dst in mig.items()
                        if dst == dev and (bb, c, pp) == (b, CLS[qb], p)]

            def vtile(b, h, t):
                if ("v", b, h, t) not in val:
                    r = pl.ds(64 * h, 64)
                    if t == (0, 3):
                        v = jnp.where(left, vb[b, r, pl.ds(0, 128)], vb[b, r, pl.ds(128, 128)])
                    else:
                        v = vb[b, r, pl.ds(64 * t[0], 128)]
                    val["v", b, h, t] = v.astype(BF16)
                return val["v", b, h, t]

            def set_q(u, q):
                val["q", u] = jnp.concatenate(
                    [jnp.where(left, q, 0.0), jnp.where(left, 0.0, q)], axis=0).astype(BF16)

            def get_set(u, h, chips):
                d = acc[u, h]
                if chips not in d:
                    rem, keys = set(chips), []
                    for key in sorted(d, key=lambda z: (-len(z), sorted(z))):
                        if key <= rem:
                            keys.append(key)
                            rem -= key
                    assert not rem
                    if ("w", u, tuple(keys)) not in val:
                        val["w", u, tuple(keys)], lse = merge_weights([lses[u, z] for z in keys])
                        lses.setdefault((u, chips), lse)
                    terms = [d[z] * w for z, w in zip(keys, val["w", u, tuple(keys)])]
                    d[chips] = sum(terms[1:], terms[0])
                return d[chips]

            def put(i, t, row=8):
                stores.setdefault(i, []).append((row, pltpu.bitcast(t, U32)))

            for op in plan["prog"][dev]:
                k = op[0]
                if k == "bar":
                    if dev in (1, 3):
                        pl.semaphore_wait(dsem, 1)
                    else:
                        pl.semaphore_wait(bar, 2)
                    if dev == 2:
                        for d in (1, 3, 0) if d0sig else (1, 3):
                            sig(dsem, d)
                elif k == "bard":
                    pl.semaphore_wait(dsem, 1)
                elif k == "fence":
                    pl.semaphore_wait(fsem, 1)
                elif k == "wait":
                    wait_rows(lsem.at[lsem_of[dev, op[1][0]]], 2 * sum(kib(n) for n in op[1]))
                elif k == "rwait":
                    wait_rows(rsem.at[rsem_of[op[1][0]]], sum(rows_of(msgs[i])[1] for i in op[1]))
                elif k == "start":
                    for row, t in stores.pop(op[1], ()):
                        sbuf[pl.ds(40 * sslot[route(msgs[op[1]])] + row, t.shape[0]), :] = t
                    rdma(op[1]).start()
                elif k == "wocast":
                    for hh in range(2):
                        val["wo", hh] = jnp.concatenate(
                            [wob[pl.ds(64 * hh, 64), :], wob[pl.ds(128 + 64 * hh, 64), :]],
                            axis=0).astype(BF16)
                elif k == "kprep":
                    _, b, p, t = op
                    c = pl.ds(0, 256) if t is None else pl.ds(128 * t, 128)
                    kk = kb[b, pl.ds(128 * p, 128), c].T
                    for i, j in enumerate(range(4) if t is None else (2 * t, 2 * t + 1)):
                        val["k", b, p, j] = kk[64 * i:64 * i + 64].astype(BF16)
                elif k == "q":
                    _, b, qb, p = op
                    if ("x", b, qb) not in val:
                        val["x", b, qb] = xb[b, pl.ds(64 * qb, 64), :].astype(BF16)
                    if ("wq", p) not in val:
                        val["wq", p] = wqb[:, pl.ds(128 * p, 128)].astype(BF16)
                    q = dot(val["x", b, qb], val["wq", p], NN) * QSCALE
                    val["qf", op[1:]] = q
                    set_q(op[1:], q)
                elif k == "s":
                    u = op[1:]
                    b, qb, p = u
                    blks = list(own_blks(dev, qb))
                    for g in guests(*u):
                        blks += [(g, j) for j in own_blks(g, qb)]
                    if len(blks) <= SSPLIT:
                        s = [jnp.concatenate([dot(val["k", b, p, j][:32], val["q", u], NT),
                                              dot(val["k", b, p, j][32:], val["q", u], NT)], axis=0)
                             for j in blks]
                    else:
                        s = [dot(val["k", b, p, j], val["q", u], NT) for j in blks]
                    mx = s[0]
                    for t in s[1:]:
                        mx = jnp.maximum(mx, t)
                    m = jnp.max(mx, axis=0, keepdims=True)
                    ps = [jnp.exp2(t - m) for t in s]
                    sm = ps[0]
                    for t in ps[1:]:
                        sm = sm + t
                    l = jnp.sum(sm, axis=0, keepdims=True)
                    pd = dict(zip(blks, ps))
                    wide, packed = [], []
                    for t in pv_tiles(own_blks(dev, qb)):
                        wide.append((t, [pd.get(t[0], zero), pd.get(t[1], zero)]))
                    for g in guests(*u):
                        js = own_blks(g, qb)
                        if len(js) == 2:
                            wide.append(((g, js), [pd[g, js[0]], pd[g, js[1]]]))
                        else:
                            pj = pd[g, js[0]]
                            halves = [jnp.where(left, pj, 0.0), jnp.where(left, 0.0, pj)]
                            packed.append(((g, js), halves[::-1] if js[0] % 2 else halves))
                    cat = lambda z: [(t, jnp.concatenate(w, axis=0).astype(BF16)) for t, w in z]
                    val["p", u] = (cat(wide), cat(packed), 1.0 / l, m + jnp.log2(l))
                elif k == "pv":
                    u = op[1:]
                    b, qb, p = u
                    wide, packed, inv, lse = val["p", u]
                    split = 2 * len(wide) + len(packed) <= 2

                    def mm(a, w):
                        if split:
                            return jnp.concatenate([dot(a[:32], w, NN), dot(a[32:], w, NN)], axis=0)
                        return dot(a, w, NN)

                    ys = []
                    for hh in range(2):
                        y = None
                        for t, w in wide:
                            z = mm(vtile(b, 2 * p + hh, t), w)
                            y = z if y is None else y + z
                        ys.append(y)
                    o = jnp.where(left, ys[0], ys[1])
                    for t, w in packed:
                        o = o + mm(val["v", b, p, t], w)
                    o = o * inv
                    lses[u, frozenset([dev])] = lse
                    for h in range(4):
                        acc.setdefault((u, h), {})[frozenset([dev])] = o[16 * h:16 * h + 16]
                elif k == "prep":
                    _, i, h = op
                    m = msgs[i]
                    b, p, kind = m["b"], m["p"], m["set"]
                    u = (b, m["q"], p)
                    if kind == "Q":
                        put(i, val["qf", u].astype(BF16))
                    elif kind in KVS:
                        js = own_blks(dev, m["q"])
                        n = int(kind[1:] or 0)
                        if kind[0] == "K":
                            put(i, val["k", b, p, js[n]])
                        elif len(js) == 2:
                            put(i, vtile(b, 2 * p + n, js))
                        else:
                            c = pl.ds(128 * (js[0] // 2), 128)
                            v0 = vb[b, pl.ds(128 * p, 64), c]
                            v1 = pltpu.roll(vb[b, pl.ds(128 * p + 64, 64), c], 64, 1)
                            put(i, jnp.where(left == (js[0] % 2 == 0), v0, v1).astype(BF16))
                    elif kind != "T":
                        put(i, get_set(u, h, kind).astype(BF16), row_of(m, h))
                        if row_of(m, h) == 8:
                            put(i, lses[u, kind], 7)
                    elif u + (h,) not in got:
                        put(i, get_set(u, h, contrib(*u)).astype(BF16), row_of(m, h))
                elif k == "recv":
                    _, i, h = op
                    m = msgs[i]
                    b, p, kind = m["b"], m["p"], m["set"]
                    u = (b, m["q"], p)
                    slot = rslot[route(m)]
                    rows = pl.ds(8, 32) if h is None else pl.ds(row_of(m, h), 8)
                    t = pltpu.bitcast(rbuf[slot, rows, :], BF16)
                    if kind == "Q":
                        set_q(u, t.astype(F32))
                    elif kind in KVS:
                        js = own_blks(m["src"], m["q"])
                        n = int(kind[1:] or 0)
                        if kind[0] == "K":
                            val["k", b, p, (m["src"], js[n])] = t
                        elif len(js) == 2:
                            val["v", b, 2 * p + n, (m["src"], js)] = t
                        else:
                            val["v", b, p, (m["src"], js)] = t
                    elif kind == "T":
                        acc.setdefault((u, h), {})[contrib(*u)] = t.astype(F32)
                    else:
                        if (u, kind) not in lses:
                            lses[u, kind] = pltpu.bitcast(rbuf[slot, pl.ds(7, 1), :], F32)
                        acc.setdefault((u, h), {})[kind] = t.astype(F32)
                elif k == "ctx":
                    _, b, qb = op
                    c = jnp.concatenate([get_set((b, qb, p), h, contrib(b, qb, p))
                                         for p in range(2) for h in range(4)], axis=0).T
                    val["ctx", b, qb] = (c[:64].astype(BF16), c[64:].astype(BF16))
                elif k == "out":
                    _, b, qb = op
                    c = val["ctx", b, qb]
                    y = dot(c[0], val["wo", 0], NN)
                    o_ref[b, pl.ds(64 * qb, 64), :] = dot(c[1], val["wo", 1], NN) + y
                else:
                    raise ValueError(op)
            wait_rows(ssem, sum(rows_of(m)[1] for m in msgs if m["src"] == dev))

        for dev in BRANCH_ORDER:
            pl.when(my == dev)(lambda dev=dev: run(dev))

    def kernel(x, Wq, K_ext, V_ext, Wo):
        kt = jnp.transpose(K_ext, (0, 2, 3, 1)).reshape(2, 256, 256)
        vt = jnp.transpose(V_ext, (0, 2, 3, 1)).reshape(2, 256, 256)
        return pl.pallas_call(
            body,
            out_shape=jax.ShapeDtypeStruct((2, 256, 512), F32),
            in_specs=[pl.BlockSpec(memory_space=pl.ANY)] * 5,
            out_specs=pl.BlockSpec(memory_space=pltpu.VMEM),
            scratch_shapes=[
                pltpu.VMEM((2, 256, 512), F32), pltpu.VMEM((512, 256), F32),
                pltpu.VMEM((2, 256, 256), F32), pltpu.VMEM((2, 256, 256), F32),
                pltpu.VMEM((256, 512), F32),
                pltpu.VMEM((n_sbuf * 40, 128), U32), pltpu.VMEM((n_rbuf, 40, 128), U32),
                pltpu.VMEM((2048, 128), U32),
                pltpu.SemaphoreType.DMA((n_load,)), pltpu.SemaphoreType.DMA,
                pltpu.SemaphoreType.DMA((n_recv,)),
                pltpu.SemaphoreType.REGULAR, pltpu.SemaphoreType.REGULAR,
            ],
            compiler_params=pltpu.CompilerParams(collective_id=0, disable_semaphore_checks=True),
        )(x, Wq, kt, vt, Wo)

    return kernel


_MSGS = [(0, 1, 1, 2, 0, None, 'Q'), (0, 1, 0, 2, 1, None, 'Q'), (0, 1, 1, 2, 1, None, 'Q'),
 (0, 1, 0, 3, 1, None, 'Q'), (0, 3, 0, 2, 0, None, 'Q'), (0, 3, 0, 2, 1, None, 'Q'),
 (0, 3, 0, 3, 1, None, 'Q'), (1, 0, 1, 0, 0, None, 'K'), (1, 0, 1, 0, 0, None, 'V'),
 (1, 0, 1, 0, 1, None, 'K'), (1, 0, 1, 0, 1, None, 'V'), (1, 0, 0, 0, 0, None, 'K'),
 (1, 0, 0, 0, 0, None, 'V'), (1, 2, 1, 1, 0, None, 'K'), (1, 2, 1, 1, 0, None, 'V'),
 (2, 0, 0, 0, 0, None, 'K'), (2, 0, 0, 0, 0, None, 'V'), (2, 1, 0, 0, 1, None, 'K'),
 (2, 1, 0, 0, 1, None, 'V'), (2, 3, 1, 0, 1, None, 'K'), (2, 3, 1, 0, 1, None, 'V'),
 (2, 3, 1, 0, 0, None, 'K'), (2, 3, 1, 0, 0, None, 'V'), (2, 3, 0, 2, 1, None, 'K'),
 (2, 3, 0, 2, 1, None, 'V'), (3, 0, 0, 1, 0, None, 'K'), (3, 0, 0, 1, 0, None, 'V'),
 (3, 0, 0, 0, 0, None, 'K0'), (3, 0, 0, 0, 0, None, 'K1'), (3, 0, 0, 0, 0, None, 'V0'),
 (3, 0, 0, 0, 0, None, 'V1'), (3, 2, 0, 1, 1, None, 'K'), (3, 2, 0, 1, 1, None, 'V'),
 (3, 2, 1, 2, 1, None, 'K'), (3, 2, 1, 2, 1, None, 'V'), (0, 3, 0, 2, 0, (0,), (0,)),
 (0, 3, 0, 2, 0, (1,), (0,)), (0, 3, 0, 2, 0, (3,), (0,)), (0, 3, 0, 2, 0, (2,), (0,)),
 (0, 3, 1, 2, 0, (0,), (0,)), (0, 3, 1, 1, 0, (2,), (0,)), (0, 3, 1, 1, 0, (1,), (0,)),
 (0, 3, 1, 1, 0, (0,), (0,)), (0, 3, 1, 2, 0, (1,), (0,)), (0, 1, 1, 2, 1, (0,), (0,)),
 (0, 3, 1, 1, 0, (3,), (0,)), (0, 1, 1, 2, 1, (2,), (0,)), (0, 2, 1, 1, 1, (1,), (0,)),
 (0, 1, 1, 2, 1, (1,), (0,)), (0, 2, 1, 1, 1, (0,), (0,)), (0, 1, 0, 1, 0, (0,), (0,)),
 (0, 1, 0, 1, 0, (1,), (0,)), (0, 3, 1, 3, 0, (0,), (0,)), (0, 3, 1, 3, 0, (1,), (0,)),
 (0, 1, 1, 2, 1, (3,), (0,)), (0, 1, 0, 1, 0, (2,), (0,)), (0, 2, 1, 1, 1, (2,), (0,)),
 (0, 3, 1, 3, 0, (3,), (0,)), (0, 3, 1, 3, 0, (2,), (0,)), (0, 2, 1, 1, 1, (3,), (0,)),
 (0, 3, 1, 2, 0, (2,), (0,)), (0, 3, 1, 2, 0, (3,), (0,)), (0, 1, 0, 1, 0, (3,), (0,)),
 (0, 1, 0, 1, 1, (0,), (0,)), (0, 1, 0, 1, 1, (1,), (0,)), (0, 1, 0, 1, 1, (2,), (0,)),
 (0, 3, 0, 2, 1, (0,), (0,)), (0, 1, 0, 1, 1, (3,), (0,)), (0, 3, 0, 2, 1, (3,), (0,)),
 (0, 3, 0, 2, 1, (2,), (0,)), (0, 3, 0, 2, 1, (1,), (0,)), (0, 3, 1, 0, 1, (0,), (0,)),
 (0, 3, 1, 0, 1, (3,), (0,)), (0, 1, 1, 3, 1, (3,), (0,)), (0, 3, 1, 3, 1, (1,), (0,)),
 (0, 1, 0, 0, 1, (0,), (0, 3)), (0, 3, 1, 0, 0, (2,), (0,)), (0, 3, 1, 0, 0, (3,), (0,)),
 (0, 3, 1, 0, 1, (1,), (0,)), (0, 1, 0, 0, 1, (1,), (0, 3)), (0, 3, 1, 0, 0, (0,), (0,)),
 (0, 1, 0, 3, 1, (1,), (0, 3)), (0, 3, 1, 0, 1, (2,), (0,)), (0, 1, 0, 3, 1, (0,), (0, 3)),
 (0, 1, 0, 3, 1, (3,), (0, 3)), (0, 3, 1, 0, 0, (1,), (0,)), (0, 1, 0, 3, 0, (2,), 'T'),
 (0, 3, 0, 3, 0, (0,), 'T'), (0, 1, 0, 0, 0, (3,), 'T'), (0, 1, 0, 3, 0, (0,), 'T'),
 (0, 3, 0, 3, 0, (2,), 'T'), (0, 1, 0, 3, 0, (3,), 'T'), (0, 3, 0, 0, 0, (3,), 'T'),
 (0, 3, 0, 3, 0, (3,), 'T'), (0, 1, 0, 3, 1, (2,), 'T'), (0, 3, 0, 3, 1, (0,), 'T'),
 (0, 1, 0, 3, 0, (1,), 'T'), (0, 3, 0, 3, 1, (1,), 'T'), (0, 1, 1, 3, 1, (0,), 'T'),
 (0, 3, 0, 3, 1, (2,), (0, 1)), (0, 1, 1, 3, 1, (3,), (3,)), (0, 3, 1, 3, 1, (0,), 'T'),
 (0, 1, 0, 0, 0, (2,), 'T'), (0, 3, 0, 0, 1, (1,), (0, 1)), (0, 3, 0, 3, 0, (1,), 'T'),
 (0, 1, 0, 0, 1, (3,), 'T'), (0, 3, 0, 0, 1, (0,), (0, 1)), (0, 1, 0, 0, 0, (0,), 'T'),
 (0, 3, 1, 3, 1, (2,), 'T'), (0, 1, 0, 0, 1, (2,), 'T'), (0, 1, 1, 3, 1, (1,), 'T'),
 (0, 3, 0, 0, 0, (0,), 'T'), (0, 1, 1, 3, 1, (2,), 'T'), (0, 3, 0, 0, 1, (2,), 'T'),
 (0, 3, 0, 3, 1, (3,), 'T'), (0, 1, 0, 0, 0, (1,), 'T'), (0, 3, 0, 0, 0, (1,), 'T'),
 (0, 1, 1, 1, 1, (0,), 'T'), (0, 3, 0, 0, 0, (2,), 'T'), (0, 3, 1, 3, 1, (3,), 'T'),
 (0, 1, 1, 1, 1, (1,), 'T'), (0, 1, 1, 0, 1, (2,), 'T'), (0, 1, 1, 0, 0, (2,), 'T'),
 (0, 3, 0, 0, 1, (3,), 'T'), (0, 3, 0, 1, 1, (0,), 'T'), (0, 1, 1, 0, 1, (3,), 'T'),
 (0, 1, 1, 0, 0, (0,), 'T'), (0, 1, 1, 0, 1, (1,), 'T'), (0, 1, 1, 0, 0, (3,), 'T'),
 (0, 1, 1, 0, 1, (0,), 'T'), (0, 3, 0, 1, 1, (3,), 'T'), (0, 1, 1, 0, 0, (1,), 'T'),
 (1, 2, 1, 1, 1, (3,), (1,)), (1, 2, 1, 1, 1, (2,), (1,)), (1, 2, 1, 1, 1, (0,), (1,)),
 (1, 2, 1, 1, 1, (1,), (1,)), (1, 2, 1, 2, 0, (1,), (1,)), (1, 2, 1, 2, 0, (2,), (1,)),
 (1, 2, 1, 2, 0, (0,), (1,)), (1, 2, 1, 2, 0, (3,), (1,)), (1, 3, 0, 2, 1, (0,), (1,)),
 (1, 3, 0, 2, 1, (2,), (1,)), (1, 3, 0, 2, 1, (1,), (1,)), (1, 3, 0, 2, 1, (3,), (1,)),
 (1, 2, 0, 2, 0, (0,), (1,)), (1, 0, 0, 3, 1, (0,), (1,)), (1, 2, 0, 2, 0, (2,), (1,)),
 (1, 2, 0, 2, 0, (1,), (1,)), (1, 0, 0, 3, 1, (1,), (1,)), (1, 0, 0, 3, 1, (2, 3), (1,)),
 (1, 2, 0, 2, 0, (3,), (1,)), (1, 0, 0, 0, 1, (0,), (1,)), (1, 0, 0, 0, 1, (1,), (1,)),
 (1, 0, 0, 0, 1, (2,), (1,)), (1, 0, 0, 0, 1, (3,), (1,)), (1, 2, 1, 2, 1, (0,), (0, 1)),
 (1, 0, 0, 1, 0, (0,), 'T'), (1, 2, 0, 1, 0, (0,), (0, 1)), (1, 0, 0, 1, 0, (2,), 'T'),
 (1, 2, 0, 1, 0, (2,), (0, 1)), (1, 0, 0, 1, 0, (1,), 'T'), (1, 2, 0, 1, 0, (1,), (0, 1)),
 (1, 0, 0, 1, 0, (3,), 'T'), (1, 2, 1, 2, 1, (3,), (0, 1)), (1, 2, 1, 2, 1, (2,), (0, 1)),
 (1, 2, 0, 1, 0, (3,), (0, 1)), (1, 0, 0, 1, 1, (0,), 'T'), (1, 0, 0, 1, 1, (1,), 'T'),
 (1, 2, 0, 1, 1, (1,), 'T'), (1, 3, 0, 1, 1, (2,), 'T'), (1, 0, 0, 1, 1, (2, 3), 'T'),
 (1, 2, 1, 3, 1, (3,), (0,)), (1, 3, 0, 1, 1, (1,), 'T'), (1, 2, 0, 1, 1, (0,), 'T'),
 (1, 2, 0, 1, 1, (2,), 'T'), (1, 2, 0, 0, 1, (0,), 'T'), (1, 0, 1, 2, 1, (0,), 'T'),
 (1, 2, 0, 1, 1, (3,), 'T'), (1, 0, 1, 2, 1, (1,), 'T'), (1, 3, 1, 2, 1, (1,), 'T'),
 (1, 0, 1, 2, 1, (2,), 'T'), (1, 2, 0, 3, 1, (0,), 'T'), (1, 0, 1, 2, 1, (3,), 'T'),
 (1, 2, 0, 3, 1, (1,), 'T'), (1, 2, 0, 0, 1, (1,), 'T'), (1, 2, 0, 3, 1, (2,), 'T'),
 (1, 2, 1, 2, 1, (1,), 'T'), (1, 2, 0, 3, 0, (2,), 'T'), (1, 2, 0, 0, 0, (3,), 'T'),
 (1, 2, 0, 3, 0, (3,), 'T'), (1, 2, 0, 0, 1, (3,), 'T'), (1, 2, 0, 3, 1, (3,), 'T'),
 (1, 2, 0, 0, 1, (2,), 'T'), (1, 2, 0, 0, 0, (0,), 'T'), (1, 2, 0, 0, 0, (2,), 'T'),
 (2, 1, 0, 1, 0, (0,), (2,)), (2, 1, 0, 1, 0, (2,), (2,)), (2, 1, 0, 1, 0, (1,), (2,)),
 (2, 1, 0, 1, 0, (3,), (2,)), (2, 1, 0, 1, 1, (0,), (2,)), (2, 1, 0, 1, 1, (1,), (2,)),
 (2, 1, 0, 1, 1, (2, 3), (2,)), (2, 0, 1, 1, 1, (0,), (1, 2, 3)), (2, 0, 1, 1, 1, (1,), (1, 2, 3)),
 (2, 3, 1, 1, 0, (0,), (2,)), (2, 3, 1, 1, 0, (1,), (2,)), (2, 3, 1, 1, 0, (3,), (2,)),
 (2, 0, 1, 1, 1, (2,), (1, 2, 3)), (2, 0, 1, 1, 1, (3,), (1, 2, 3)), (2, 3, 1, 1, 0, (2,), (2,)),
 (2, 1, 1, 2, 1, (0,), (2,)), (2, 1, 1, 2, 1, (1,), (2,)), (2, 3, 1, 2, 0, (0,), (1, 2)),
 (2, 3, 1, 2, 0, (1,), (1, 2)), (2, 3, 1, 2, 0, (2,), (1, 2)), (2, 3, 1, 2, 0, (3,), (1, 2)),
 (2, 1, 1, 2, 1, (2,), (2,)), (2, 1, 1, 2, 1, (3,), (2,)), (2, 0, 0, 2, 0, (0,), 'T'),
 (2, 0, 0, 2, 0, (2,), 'T'), (2, 3, 1, 1, 1, (0,), 'T'), (2, 0, 0, 2, 0, (1,), 'T'),
 (2, 3, 1, 1, 1, (1,), 'T'), (2, 0, 0, 2, 0, (3,), 'T'), (2, 1, 0, 2, 0, (0,), 'T'),
 (2, 3, 1, 1, 1, (2,), 'T'), (2, 1, 0, 2, 0, (3,), 'T'), (2, 1, 0, 2, 0, (1,), 'T'),
 (2, 3, 0, 2, 0, (3,), (1, 2)), (2, 3, 0, 2, 0, (1,), (1, 2)), (2, 1, 1, 1, 1, (2,), (0, 2, 3)),
 (2, 3, 0, 2, 0, (0,), (1, 2)), (2, 1, 1, 1, 0, (0,), 'T'), (2, 3, 1, 1, 1, (3,), (0, 1, 2)),
 (2, 1, 1, 1, 0, (2,), 'T'), (2, 3, 0, 1, 0, (0,), 'T'), (2, 1, 1, 1, 0, (3,), 'T'),
 (2, 1, 1, 1, 1, (3,), (0, 2, 3)), (2, 3, 0, 1, 0, (1,), 'T'), (2, 1, 0, 2, 0, (2,), 'T'),
 (2, 3, 0, 2, 0, (2,), (1, 2)), (2, 1, 1, 3, 0, (1,), 'T'), (2, 1, 1, 1, 0, (1,), 'T'),
 (2, 1, 1, 3, 0, (0,), 'T'), (2, 1, 1, 3, 0, (2,), 'T'), (2, 3, 1, 2, 1, (3,), 'T'),
 (2, 3, 0, 1, 0, (2,), 'T'), (2, 3, 1, 2, 1, (0,), 'T'), (2, 1, 1, 2, 0, (1,), (0, 2, 3)),
 (2, 1, 1, 2, 0, (2,), 'T'), (2, 3, 1, 2, 1, (2,), 'T'), (2, 1, 1, 2, 0, (0,), 'T'),
 (2, 1, 1, 3, 0, (3,), 'T'), (2, 1, 1, 2, 0, (3,), 'T'), (2, 1, 0, 2, 1, (0,), 'T'),
 (2, 3, 0, 1, 0, (3,), 'T'), (2, 1, 0, 2, 1, (1,), 'T'), (2, 1, 0, 2, 1, (3,), 'T'),
 (2, 1, 0, 2, 1, (2,), 'T'), (3, 2, 1, 1, 1, (0,), (3,)), (3, 2, 1, 1, 1, (2,), (3,)),
 (3, 2, 1, 1, 1, (3,), (3,)), (3, 2, 1, 1, 1, (1,), (3,)), (3, 0, 0, 0, 1, (0,), (3,)),
 (3, 0, 0, 0, 1, (1,), (3,)), (3, 0, 0, 3, 1, (0,), (3,)), (3, 0, 0, 3, 1, (1,), (3,)),
 (3, 0, 0, 0, 1, (3,), (3,)), (3, 0, 0, 3, 1, (2,), (3,)), (3, 2, 0, 2, 0, (0,), (0, 3)),
 (3, 0, 0, 3, 1, (3,), (3,)), (3, 2, 0, 2, 0, (3,), (0, 3)), (3, 0, 0, 0, 1, (2,), (3,)),
 (3, 2, 0, 2, 0, (2,), (0, 3)), (3, 0, 1, 0, 1, (0,), (3,)), (3, 2, 0, 2, 0, (1,), (0, 3)),
 (3, 0, 1, 0, 1, (3,), (3,)), (3, 0, 1, 0, 1, (2,), (3,)), (3, 0, 1, 0, 1, (1,), (3,)),
 (3, 2, 1, 1, 0, (0,), (0,)), (3, 0, 1, 3, 1, (3,), (3,)), (3, 0, 1, 3, 1, (0,), (3,)),
 (3, 2, 1, 3, 1, (3,), (3,)), (3, 0, 1, 3, 1, (2,), (3,)), (3, 2, 1, 1, 0, (1,), (0,)),
 (3, 0, 1, 3, 1, (1,), (3,)), (3, 0, 1, 0, 0, (3,), (3,)), (3, 2, 1, 1, 0, (0,), (3,)),
 (3, 2, 1, 1, 0, (2,), (0, 3)), (3, 0, 1, 0, 0, (1,), (3,)), (3, 2, 1, 1, 0, (3,), (0, 3)),
 (3, 2, 1, 1, 0, (1,), (3,)), (3, 0, 1, 0, 0, (0,), (3,)), (3, 0, 1, 0, 0, (2,), (3,)),
 (3, 0, 1, 3, 0, (0,), 'T'), (3, 2, 1, 3, 0, (1,), 'T'), (3, 0, 1, 3, 0, (3,), 'T'),
 (3, 2, 1, 3, 0, (0,), 'T'), (3, 0, 1, 3, 0, (2,), 'T'), (3, 2, 1, 3, 0, (2,), 'T'),
 (3, 2, 1, 2, 0, (0,), (0, 3)), (3, 2, 1, 2, 0, (1,), (0, 3)), (3, 0, 1, 3, 0, (1,), 'T'),
 (3, 0, 0, 2, 1, (0,), (1, 3)), (3, 2, 1, 2, 0, (2,), (0, 3)), (3, 2, 0, 2, 1, (0,), 'T'),
 (3, 2, 1, 3, 0, (3,), 'T'), (3, 0, 0, 2, 1, (2,), (1, 3)), (3, 2, 1, 2, 0, (3,), (0, 3)),
 (3, 0, 0, 2, 1, (3,), (1, 3)), (3, 2, 0, 2, 1, (2,), (1, 3)), (3, 0, 0, 2, 1, (1,), (1, 3)),
 (3, 0, 1, 1, 0, (0,), 'T'), (3, 0, 1, 1, 0, (1,), 'T'), (3, 2, 0, 2, 1, (1,), 'T'),
 (3, 0, 1, 1, 0, (3,), 'T'), (3, 0, 1, 1, 0, (2,), 'T'), (3, 2, 0, 2, 1, (2,), (0,)),
 (3, 0, 1, 2, 0, (0,), 'T'), (3, 2, 0, 2, 1, (3,), 'T'), (3, 0, 1, 2, 0, (1,), 'T'),
 (3, 2, 1, 0, 0, (0,), 'T'), (3, 0, 1, 2, 0, (2,), 'T'), (3, 2, 1, 0, 1, (0,), 'T'),
 (3, 2, 1, 0, 1, (3,), 'T'), (3, 0, 1, 2, 0, (3,), 'T'), (3, 2, 1, 0, 1, (2,), 'T'),
 (3, 2, 0, 3, 0, (0,), 'T'), (3, 2, 1, 0, 0, (3,), 'T'), (3, 2, 1, 0, 0, (1,), 'T'),
 (3, 2, 1, 0, 0, (2,), 'T'), (3, 2, 1, 0, 1, (1,), 'T'), (3, 2, 0, 3, 0, (1,), 'T'),
 (3, 2, 1, 3, 1, (0,), 'T'), (3, 2, 1, 3, 1, (1,), 'T'), (3, 2, 1, 3, 1, (2,), 'T'),
 (3, 2, 0, 0, 0, (1,), 'T')]

_LOADS = {0: [('x', 0, 2), ('wq', 0), ('x', 1, 2), ('x', 0, 3), ('wq', 1), ('k', 1, 0, None),
     ('k', 0, 0, None), ('x', 1, 1), ('v', 0, 0, None), ('k', 1, 1, None), ('v', 1, 0, None),
     ('x', 0, 1), ('v', 1, 1, None), ('x', 1, 3), ('k', 0, 1, None), ('x', 1, 0), ('x', 0, 0),
     ('v', 0, 1, None), ('wo',)],
 1: [('v', 1, 0, 1), ('k', 1, 0, 1), ('v', 1, 1, 1), ('k', 1, 1, 1), ('v', 1, 0, 0), ('k', 0, 0, 1),
     ('k', 1, 0, 0), ('k', 1, 1, 0), ('x', 1, 1), ('wq', 1), ('k', 0, 1, 1), ('v', 1, 1, 0),
     ('v', 0, 0, 1), ('k', 0, 1, 0), ('v', 0, 1, 0), ('v', 0, 1, 1), ('k', 0, 0, 0), ('x', 0, 2),
     ('wq', 0), ('x', 0, 0), ('v', 0, 0, 0), ('x', 0, 1), ('wo',)],
 2: [('k', 1, 1, 0), ('k', 0, 1, 0), ('v', 1, 1, 0), ('k', 1, 0, 0), ('v', 0, 1, 0), ('k', 0, 0, 1),
     ('k', 0, 0, 0), ('v', 1, 0, 0), ('v', 0, 0, 0), ('x', 0, 1), ('wq', 0), ('k', 0, 1, 1),
     ('v', 0, 0, 1), ('v', 0, 1, 1), ('wq', 1), ('x', 1, 1), ('k', 1, 0, 1), ('k', 1, 1, 1),
     ('x', 1, 2), ('x', 0, 2), ('v', 1, 0, 1), ('v', 1, 1, 1), ('wo',)],
 3: [('v', 0, 0, 1), ('k', 0, 0, 1), ('k', 1, 1, 0), ('v', 0, 0, 0), ('k', 0, 1, 1), ('k', 1, 1, 1),
     ('x', 1, 1), ('k', 0, 1, 0), ('v', 0, 1, 1), ('wq', 1), ('k', 0, 0, 0), ('x', 0, 0),
     ('v', 1, 1, 1), ('v', 1, 0, 0), ('v', 1, 1, 0), ('v', 0, 1, 0), ('x', 1, 0), ('x', 1, 3),
     ('k', 1, 0, 1), ('k', 1, 0, 0), ('wq', 0), ('x', 1, 2), ('v', 1, 0, 1), ('wo',)]}

_PROG = {0: [('wait', (('x', 1, 2), ('wq', 0))), ('q', 1, 2, 0), ('wait', (('x', 0, 2),)), ('q', 0, 2, 0),
     ('bar',), ('wait', (('x', 0, 3),)), ('prep', 4, None), ('prep', 0, None), ('start', 4),
     ('start', 0), ('wait', (('wq', 1),)), ('q', 0, 2, 1), ('q', 0, 3, 1),
     ('wait', (('k', 1, 0, None),)), ('prep', 6, None), ('prep', 1, None), ('prep', 5, None),
     ('start', 6), ('start', 1), ('start', 5), ('wait', (('k', 0, 0, None),)), ('prep', 3, None),
     ('start', 3), ('wait', (('x', 1, 1),)), ('q', 1, 1, 0), ('q', 1, 2, 1), ('kprep', 0, 0, None),
     ('kprep', 1, 0, None), ('prep', 2, None), ('s', 1, 2, 0), ('q', 1, 1, 1), ('s', 0, 2, 0),
     ('s', 1, 1, 0), ('start', 2),
     ('wait', (('k', 1, 1, None), ('v', 1, 0, None), ('v', 0, 0, None))), ('pv', 0, 2, 0),
     ('prep', 35, 0), ('pv', 1, 2, 0), ('kprep', 1, 1, None), ('prep', 36, 1), ('prep', 37, 3),
     ('start', 35), ('start', 36), ('start', 37), ('wait', (('x', 0, 1),)), ('prep', 38, 2),
     ('q', 0, 1, 0), ('pv', 1, 1, 0), ('prep', 39, 0), ('s', 1, 2, 1), ('s', 1, 1, 1),
     ('prep', 40, 2), ('q', 0, 3, 0), ('prep', 41, 1), ('start', 38), ('start', 39), ('start', 40),
     ('start', 41), ('wait', (('x', 1, 3),)), ('rwait', (26, 8)), ('prep', 42, 0), ('start', 42),
     ('wait', (('v', 1, 1, None),)), ('pv', 1, 2, 1), ('pv', 1, 1, 1), ('prep', 43, 1),
     ('q', 0, 1, 1), ('q', 1, 3, 0), ('prep', 44, 0), ('prep', 45, 3), ('start', 43), ('start', 44),
     ('start', 45), ('bard',), ('wait', (('k', 0, 1, None),)), ('prep', 46, 2), ('prep', 47, 1),
     ('start', 46), ('start', 47), ('rwait', (7,)), ('prep', 48, 1), ('prep', 49, 0), ('start', 48),
     ('start', 49), ('rwait', (25,)), ('recv', 25, None), ('s', 0, 1, 0), ('kprep', 0, 1, None),
     ('recv', 7, None), ('s', 1, 3, 0), ('s', 0, 1, 1), ('recv', 26, None), ('pv', 0, 1, 0),
     ('recv', 8, None), ('pv', 1, 3, 0), ('prep', 50, 0), ('prep', 51, 1), ('prep', 52, 0),
     ('prep', 53, 1), ('start', 50), ('start', 51), ('start', 52), ('start', 53),
     ('wait', (('v', 0, 1, None), ('x', 0, 0))), ('prep', 54, 3), ('start', 54),
     ('wait', (('x', 1, 0),)), ('prep', 55, 2), ('prep', 56, 2), ('start', 55), ('start', 56),
     ('rwait', (10,)), ('s', 0, 2, 1), ('prep', 57, 3), ('prep', 58, 2), ('pv', 0, 1, 1),
     ('prep', 59, 3), ('q', 1, 0, 0), ('prep', 60, 2), ('prep', 61, 3), ('prep', 62, 3),
     ('q', 1, 0, 1), ('prep', 63, 0), ('prep', 64, 1), ('q', 1, 3, 1), ('start', 57), ('start', 58),
     ('start', 59), ('start', 60), ('start', 61), ('start', 62), ('start', 63), ('start', 64),
     ('rwait', (9,)), ('pv', 0, 2, 1), ('prep', 65, 2), ('prep', 66, 0), ('recv', 9, None),
     ('s', 1, 3, 1), ('s', 1, 0, 1), ('s', 1, 0, 0), ('prep', 67, 3), ('q', 0, 0, 1),
     ('prep', 68, 3), ('s', 0, 0, 1), ('recv', 10, None), ('pv', 1, 0, 1), ('prep', 69, 2),
     ('pv', 1, 3, 1), ('pv', 0, 0, 1), ('prep', 70, 1), ('prep', 71, 0), ('prep', 72, 3),
     ('s', 0, 3, 1), ('pv', 1, 0, 0), ('prep', 73, 3), ('start', 65), ('start', 66), ('start', 67),
     ('start', 68), ('start', 69), ('start', 70), ('start', 71), ('start', 72), ('start', 73),
     ('rwait', (263,)), ('prep', 74, 1), ('start', 74), ('fence',), ('pv', 0, 3, 1),
     ('recv', 263, 0), ('prep', 75, 0), ('prep', 76, 2), ('q', 0, 0, 0), ('prep', 77, 3),
     ('prep', 78, 1), ('start', 75), ('start', 76), ('start', 77), ('start', 78),
     ('rwait', (15, 264)), ('recv', 264, 1), ('prep', 79, 1), ('start', 79),
     ('rwait', (30, 265, 27, 266, 11)), ('prep', 80, 0), ('recv', 266, 1), ('prep', 81, 1),
     ('prep', 82, 2), ('recv', 265, 0), ('prep', 83, 0), ('start', 80), ('start', 81),
     ('start', 82), ('start', 83), ('rwait', (29, 28)), ('recv', 11, None), ('recv', 15, None),
     ('recv', 27, None), ('recv', 28, None), ('s', 0, 0, 0), ('s', 0, 3, 0),
     ('rwait', (270, 272, 12)), ('recv', 270, 3), ('prep', 84, 3), ('prep', 85, 1), ('start', 84),
     ('start', 85), ('rwait', (16,)), ('recv', 12, None), ('recv', 16, None), ('recv', 29, None),
     ('recv', 30, None), ('pv', 0, 3, 0), ('prep', 86, 2), ('prep', 87, 0), ('pv', 0, 0, 0),
     ('start', 86), ('start', 87), ('fence',), ('prep', 88, 3), ('prep', 89, 0), ('start', 88),
     ('start', 89), ('rwait', (145,)), ('prep', 90, 2), ('start', 90), ('wait', (('wo',),)),
     ('rwait', (274, 148, 268)), ('prep', 91, 3), ('prep', 92, 3), ('prep', 93, 3), ('start', 91),
     ('start', 92), ('start', 93), ('rwait', (149,)), ('recv', 149, 2), ('recv', 268, 2),
     ('prep', 94, 2), ('recv', 145, 0), ('prep', 95, 0), ('start', 94), ('start', 95),
     ('rwait', (281,)), ('prep', 96, 1), ('start', 96), ('rwait', (151,)), ('recv', 148, 1),
     ('prep', 97, 1), ('start', 97), ('rwait', (153, 277)), ('recv', 281, 0), ('prep', 98, 0),
     ('prep', 99, 2), ('wocast',), ('start', 98), ('start', 99), ('rwait', (280,)),
     ('recv', 280, 3), ('prep', 100, 3), ('prep', 101, 0), ('prep', 102, 2), ('start', 100),
     ('start', 101), ('start', 102), ('rwait', (267, 154, 152)), ('recv', 152, 1), ('prep', 103, 1),
     ('start', 103), ('rwait', (285,)), ('prep', 104, 1), ('recv', 154, 3), ('recv', 267, 3),
     ('prep', 105, 3), ('start', 104), ('start', 105), ('rwait', (283,)), ('recv', 151, 0),
     ('prep', 106, 0), ('prep', 107, 0), ('recv', 153, 2), ('recv', 272, 2), ('ctx', 0, 0),
     ('recv', 283, 2), ('prep', 108, 2), ('prep', 109, 2), ('recv', 149, 3), ('ctx', 0, 3),
     ('recv', 285, 1), ('prep', 110, 1), ('prep', 111, 0), ('start', 106), ('start', 107),
     ('start', 108), ('start', 109), ('start', 110), ('start', 111), ('rwait', (292,)),
     ('prep', 112, 2), ('start', 112), ('rwait', (293,)), ('prep', 113, 2), ('start', 113),
     ('rwait', (202, 162)), ('prep', 114, 3), ('prep', 115, 1), ('out', 0, 3), ('prep', 116, 1),
     ('recv', 202, 0), ('prep', 117, 0), ('prep', 118, 2), ('prep', 119, 3), ('start', 114),
     ('start', 115), ('start', 116), ('start', 117), ('start', 118), ('start', 119),
     ('rwait', (303, 203, 298)), ('recv', 203, 1), ('prep', 120, 1), ('start', 120),
     ('rwait', (302, 286, 278)), ('recv', 277, 2), ('prep', 121, 2), ('recv', 293, 2),
     ('prep', 122, 2), ('start', 121), ('start', 122), ('rwait', (160, 166, 289, 276)),
     ('prep', 123, 3), ('prep', 124, 0), ('recv', 276, 3), ('prep', 125, 3), ('start', 123),
     ('start', 124), ('start', 125), ('fence',), ('recv', 292, 0), ('prep', 126, 0), ('start', 126),
     ('rwait', (296, 208, 156, 294, 167)), ('recv', 278, 1), ('prep', 127, 1), ('recv', 289, 1),
     ('recv', 286, 3), ('recv', 274, 0), ('ctx', 1, 0), ('out', 0, 0), ('recv', 294, 0),
     ('recv', 302, 1), ('recv', 298, 2), ('recv', 296, 3), ('ctx', 1, 3), ('out', 1, 0),
     ('start', 127), ('rwait', (312, 170)), ('prep', 128, 3), ('prep', 129, 0), ('prep', 130, 3),
     ('start', 128), ('start', 129), ('start', 130), ('rwait', (158,)), ('prep', 131, 1),
     ('start', 131), ('rwait', (307, 309)), ('out', 1, 3), ('recv', 156, 0), ('recv', 160, 1),
     ('recv', 158, 2), ('recv', 162, 3), ('recv', 166, 0), ('recv', 167, 1), ('recv', 170, 2),
     ('recv', 170, 3), ('ctx', 0, 1), ('rwait', (316, 223, 315, 313, 207, 221, 311, 218, 219)),
     ('out', 0, 1), ('recv', 312, 0), ('recv', 313, 1), ('recv', 316, 2), ('recv', 315, 3),
     ('recv', 207, 2), ('recv', 208, 3), ('ctx', 1, 1), ('recv', 218, 0), ('recv', 221, 1),
     ('recv', 219, 2), ('recv', 223, 3), ('recv', 303, 0), ('recv', 311, 1), ('recv', 307, 2),
     ('recv', 309, 3), ('ctx', 0, 2), ('out', 1, 1),
     ('rwait', (320, 180, 325, 178, 318, 176, 322, 182)), ('recv', 318, 0), ('recv', 320, 1),
     ('recv', 322, 2), ('recv', 325, 3), ('recv', 176, 0), ('recv', 178, 1), ('recv', 180, 2),
     ('recv', 182, 3), ('ctx', 1, 2), ('out', 0, 2), ('out', 1, 2)],
 1: [('wait', (('v', 1, 0, 1),)), ('prep', 8, None), ('start', 8),
     ('wait', (('v', 1, 1, 1), ('k', 1, 0, 1), ('k', 1, 1, 1))), ('kprep', 1, 0, 1),
     ('prep', 7, None), ('start', 7), ('wait', (('v', 1, 0, 0),)), ('prep', 10, None),
     ('start', 10), ('wait', (('k', 1, 0, 0),)), ('kprep', 1, 0, 0), ('kprep', 1, 1, 1),
     ('prep', 9, None), ('start', 9), ('bar',), ('prep', 13, None), ('start', 13),
     ('wait', (('k', 0, 0, 1),)), ('kprep', 0, 0, 1), ('wait', (('k', 1, 1, 0),)),
     ('kprep', 1, 1, 0), ('wait', (('x', 1, 1),)), ('prep', 11, None), ('start', 11),
     ('wait', (('wq', 1),)), ('q', 1, 1, 1), ('prep', 14, None), ('start', 14),
     ('wait', (('v', 1, 1, 0), ('k', 0, 1, 1))), ('s', 1, 1, 1), ('rwait', (0,)),
     ('wait', (('k', 0, 1, 0), ('v', 0, 0, 1))), ('pv', 1, 1, 1), ('kprep', 0, 1, 1),
     ('prep', 132, 3), ('prep', 12, None), ('kprep', 0, 1, 0), ('prep', 133, 2), ('recv', 0, None),
     ('s', 1, 2, 0), ('prep', 134, 0), ('start', 132), ('start', 12), ('start', 133),
     ('start', 134), ('rwait', (1,)), ('pv', 1, 2, 0), ('prep', 135, 1), ('start', 135),
     ('wait', (('v', 0, 1, 1),)), ('prep', 136, 1), ('prep', 137, 2), ('start', 136),
     ('start', 137), ('wait', (('v', 0, 1, 0),)), ('prep', 138, 0), ('recv', 1, None),
     ('s', 0, 2, 1), ('start', 138), ('wait', (('x', 0, 2),)), ('pv', 0, 2, 1),
     ('wait', (('k', 0, 0, 0),)), ('prep', 139, 3), ('start', 139), ('rwait', (3,)),
     ('prep', 140, 0), ('prep', 141, 2), ('start', 140), ('start', 141), ('rwait', (17,)),
     ('prep', 142, 1), ('start', 142), ('wait', (('wq', 0),)), ('q', 0, 2, 0), ('kprep', 0, 0, 0),
     ('recv', 3, None), ('recv', 17, None), ('s', 0, 3, 1), ('prep', 143, 3), ('s', 0, 2, 0),
     ('start', 143), ('wait', (('x', 0, 0), ('v', 0, 0, 0))), ('rwait', (18,)), ('recv', 18, None),
     ('pv', 0, 3, 1), ('pv', 0, 2, 0), ('prep', 144, 0), ('prep', 145, 0), ('q', 0, 0, 1),
     ('prep', 146, 2), ('prep', 147, 1), ('prep', 148, 1), ('prep', 149, 2), ('prep', 149, 3),
     ('start', 144), ('start', 145), ('start', 146), ('start', 147), ('start', 148), ('start', 149),
     ('rwait', (44,)), ('prep', 150, 3), ('start', 150), ('wait', (('x', 0, 1),)), ('rwait', (2,)),
     ('s', 0, 0, 1), ('q', 0, 1, 0), ('q', 0, 1, 1), ('recv', 2, None), ('s', 1, 2, 1),
     ('pv', 0, 0, 1), ('prep', 151, 0), ('prep', 152, 1), ('s', 0, 1, 1), ('prep', 153, 2),
     ('prep', 154, 3), ('s', 0, 1, 0), ('pv', 1, 2, 1), ('start', 151), ('start', 152),
     ('start', 153), ('start', 154), ('rwait', (50,)), ('pv', 0, 1, 1), ('pv', 0, 1, 0),
     ('recv', 44, 0), ('prep', 155, 0), ('start', 155), ('rwait', (195,)), ('recv', 50, 0),
     ('recv', 195, 0), ('prep', 156, 0), ('start', 156), ('rwait', (196,)), ('prep', 157, 0),
     ('start', 157), ('rwait', (55, 46, 54, 51)), ('recv', 55, 2), ('recv', 196, 2),
     ('prep', 158, 2), ('start', 158), ('rwait', (197,)), ('prep', 159, 2), ('start', 159),
     ('rwait', (62,)), ('recv', 51, 1), ('recv', 197, 1), ('prep', 160, 1), ('start', 160),
     ('rwait', (198,)), ('prep', 161, 1), ('recv', 62, 3), ('recv', 198, 3), ('prep', 162, 3),
     ('start', 161), ('start', 162), ('rwait', (63,)), ('recv', 54, 3), ('prep', 163, 3),
     ('recv', 46, 2), ('prep', 164, 2), ('start', 163), ('start', 164), ('rwait', (65,)),
     ('prep', 165, 3), ('start', 165), ('rwait', (199, 64)), ('recv', 63, 0), ('recv', 199, 0),
     ('prep', 166, 0), ('start', 166), ('rwait', (200,)), ('recv', 64, 1), ('recv', 200, 1),
     ('prep', 167, 1), ('prep', 168, 1), ('start', 167), ('start', 168), ('rwait', (67, 201)),
     ('recv', 65, 2), ('recv', 201, 2), ('prep', 169, 2), ('recv', 67, 3), ('recv', 201, 3),
     ('prep', 170, 3), ('prep', 170, 2), ('start', 169), ('start', 170), ('rwait', (73,)),
     ('recv', 73, 3), ('prep', 171, 3), ('prep', 172, 1), ('start', 171), ('start', 172),
     ('rwait', (210,)), ('prep', 173, 0), ('start', 173), ('rwait', (48, 75)), ('prep', 174, 2),
     ('recv', 75, 0), ('prep', 175, 0), ('start', 174), ('start', 175), ('rwait', (79, 83)),
     ('recv', 210, 0), ('prep', 176, 0), ('start', 176), ('rwait', (81, 211)), ('prep', 177, 3),
     ('recv', 48, 1), ('recv', 211, 1), ('prep', 178, 1), ('prep', 179, 1), ('start', 177),
     ('start', 178), ('start', 179), ('rwait', (216,)), ('recv', 216, 2), ('prep', 180, 2),
     ('start', 180), ('rwait', (217, 84)), ('recv', 83, 0), ('prep', 181, 0), ('recv', 217, 3),
     ('prep', 182, 3), ('recv', 81, 1), ('prep', 183, 1), ('start', 181), ('start', 182),
     ('start', 183), ('rwait', (86,)), ('recv', 79, 1), ('prep', 184, 1), ('start', 184),
     ('rwait', (94,)), ('prep', 185, 2), ('prep', 186, 1), ('prep', 187, 2), ('start', 185),
     ('start', 186), ('start', 187), ('rwait', (88, 226)), ('ctx', 0, 1), ('prep', 188, 3),
     ('start', 188), ('wait', (('wo',),)), ('rwait', (227, 234, 91)), ('prep', 189, 3),
     ('start', 189), ('rwait', (105,)), ('prep', 190, 3), ('start', 190), ('rwait', (236,)),
     ('recv', 84, 3), ('prep', 191, 3), ('wocast',), ('start', 191), ('rwait', (109,)),
     ('prep', 192, 2), ('start', 192), ('rwait', (89, 107, 110)), ('prep', 193, 0), ('start', 193),
     ('rwait', (112, 115, 224, 102, 243, 242)), ('prep', 194, 2), ('start', 194),
     ('rwait', (96, 230, 244, 100)), ('recv', 107, 0), ('recv', 115, 1), ('recv', 102, 2),
     ('recv', 88, 3), ('recv', 109, 2), ('recv', 105, 3), ('ctx', 0, 0), ('recv', 89, 0),
     ('recv', 96, 1), ('recv', 86, 2), ('recv', 91, 3), ('recv', 94, 2), ('ctx', 0, 3),
     ('out', 0, 3), ('out', 0, 0),
     ('rwait', (241, 237, 117, 232, 249, 239, 252, 98, 120, 253, 248, 251)), ('recv', 243, 0),
     ('recv', 241, 1), ('recv', 244, 2), ('recv', 252, 3), ('recv', 98, 0), ('recv', 110, 1),
     ('recv', 112, 2), ('recv', 100, 3), ('ctx', 1, 3), ('recv', 232, 0), ('recv', 242, 1),
     ('recv', 234, 2), ('recv', 236, 3), ('recv', 117, 0), ('recv', 120, 1), ('recv', 230, 2),
     ('recv', 237, 3), ('ctx', 1, 1), ('out', 0, 1), ('recv', 251, 0), ('recv', 248, 1),
     ('recv', 249, 2), ('recv', 253, 3), ('ctx', 1, 2), ('out', 1, 3), ('out', 1, 1),
     ('rwait', (254, 125, 131, 257, 129, 126, 127, 121, 258, 122, 128, 256)), ('recv', 126, 0),
     ('recv', 131, 1), ('recv', 122, 2), ('recv', 128, 3), ('recv', 129, 0), ('recv', 127, 1),
     ('recv', 121, 2), ('recv', 125, 3), ('ctx', 1, 0), ('recv', 224, 0), ('recv', 227, 1),
     ('recv', 239, 2), ('recv', 226, 3), ('recv', 254, 0), ('recv', 256, 1), ('recv', 258, 2),
     ('recv', 257, 3), ('ctx', 0, 2), ('out', 1, 2), ('out', 0, 2), ('out', 1, 0)],
 2: [('bar',), ('wait', (('k', 1, 1, 0), ('k', 0, 1, 0))), ('kprep', 1, 1, 0), ('kprep', 0, 1, 0),
     ('prep', 17, None), ('prep', 19, None), ('start', 17), ('start', 19),
     ('wait', (('v', 1, 1, 0), ('k', 1, 0, 0))), ('prep', 20, None), ('start', 20),
     ('wait', (('v', 0, 1, 0),)), ('prep', 18, None), ('start', 18), ('wait', (('k', 0, 0, 0),)),
     ('kprep', 1, 0, 0), ('prep', 21, None), ('kprep', 0, 0, 0), ('prep', 15, None), ('start', 21),
     ('start', 15), ('wait', (('v', 1, 0, 0), ('x', 0, 1), ('v', 0, 0, 0), ('k', 0, 0, 1))),
     ('kprep', 0, 0, 1), ('prep', 22, None), ('prep', 16, None), ('start', 22), ('start', 16),
     ('wait', (('wq', 0),)), ('q', 0, 1, 0), ('wait', (('v', 0, 0, 1), ('k', 0, 1, 1))),
     ('kprep', 0, 1, 1), ('s', 0, 1, 0), ('prep', 23, None), ('pv', 0, 1, 0), ('prep', 195, 0),
     ('start', 23), ('start', 195), ('rwait', (31,)), ('prep', 196, 2), ('prep', 197, 1),
     ('start', 196), ('start', 197), ('rwait', (13,)), ('wait', (('wq', 1), ('v', 0, 1, 1))),
     ('prep', 198, 3), ('prep', 24, None), ('q', 0, 1, 1), ('start', 198), ('start', 24),
     ('wait', (('k', 1, 0, 1), ('x', 1, 1))), ('recv', 31, None), ('s', 0, 1, 1), ('q', 1, 1, 1),
     ('q', 1, 1, 0), ('kprep', 1, 0, 1), ('rwait', (33, 14, 32)),
     ('wait', (('k', 1, 1, 1), ('x', 1, 2))), ('recv', 32, None), ('pv', 0, 1, 1),
     ('kprep', 1, 1, 1), ('recv', 13, None), ('s', 1, 1, 0), ('q', 1, 2, 0), ('prep', 199, 0),
     ('prep', 200, 1), ('q', 1, 2, 1), ('prep', 201, 2), ('prep', 201, 3), ('s', 1, 1, 1),
     ('start', 199), ('start', 200), ('start', 201), ('rwait', (259, 134, 260, 262, 135)),
     ('wait', (('v', 1, 1, 1), ('x', 0, 2), ('v', 1, 0, 1))), ('pv', 1, 1, 1), ('recv', 134, 0),
     ('recv', 259, 0), ('prep', 202, 0), ('recv', 135, 1), ('recv', 262, 1), ('prep', 203, 1),
     ('recv', 14, None), ('pv', 1, 1, 0), ('prep', 204, 0), ('prep', 205, 1), ('recv', 33, None),
     ('s', 1, 2, 1), ('s', 1, 2, 0), ('start', 202), ('start', 203), ('start', 204), ('start', 205),
     ('rwait', (138, 133)), ('prep', 206, 3), ('start', 206), ('rwait', (136,)), ('recv', 133, 2),
     ('recv', 260, 2), ('prep', 207, 2), ('start', 207), ('rwait', (132, 139, 137, 261)),
     ('recv', 132, 3), ('recv', 261, 3), ('prep', 208, 3), ('prep', 209, 2), ('start', 208),
     ('start', 209), ('rwait', (34,)), ('recv', 34, None), ('pv', 1, 2, 1), ('pv', 1, 2, 0),
     ('prep', 210, 0), ('prep', 211, 1), ('recv', 138, 0), ('prep', 212, 0), ('recv', 136, 1),
     ('prep', 213, 1), ('q', 0, 2, 0), ('recv', 137, 2), ('prep', 214, 2), ('recv', 139, 3),
     ('prep', 215, 3), ('prep', 216, 2), ('prep', 217, 3), ('start', 210), ('start', 211),
     ('start', 212), ('start', 213), ('start', 214), ('start', 215), ('start', 216), ('start', 217),
     ('rwait', (269,)), ('s', 0, 2, 0), ('pv', 0, 2, 0), ('rwait', (144,)), ('recv', 144, 0),
     ('recv', 269, 0), ('prep', 218, 0), ('start', 218), ('rwait', (49, 273, 146)),
     ('recv', 146, 2), ('recv', 273, 2), ('prep', 219, 2), ('start', 219),
     ('rwait', (147, 271, 275)), ('recv', 49, 0), ('prep', 220, 0), ('recv', 147, 1),
     ('recv', 275, 1), ('prep', 221, 1), ('start', 220), ('start', 221), ('rwait', (47, 56)),
     ('recv', 47, 1), ('prep', 222, 1), ('start', 222), ('rwait', (150,)), ('recv', 150, 3),
     ('recv', 271, 3), ('prep', 223, 3), ('prep', 224, 0), ('recv', 56, 2), ('prep', 225, 2),
     ('prep', 226, 3), ('start', 223), ('start', 224), ('start', 225), ('start', 226),
     ('rwait', (279, 282)), ('prep', 227, 1), ('start', 227), ('rwait', (284,)), ('prep', 228, 3),
     ('prep', 229, 1), ('prep', 230, 2), ('prep', 231, 0), ('start', 228), ('start', 229),
     ('start', 230), ('start', 231), ('rwait', (287, 59)), ('recv', 279, 0), ('recv', 287, 0),
     ('prep', 232, 0), ('start', 232), ('rwait', (288,)), ('recv', 59, 3), ('prep', 233, 3),
     ('start', 233), ('fence',), ('recv', 288, 2), ('prep', 234, 2), ('start', 234),
     ('rwait', (157, 290)), ('recv', 157, 0), ('prep', 235, 0), ('recv', 290, 3), ('prep', 236, 3),
     ('prep', 237, 3), ('start', 235), ('start', 236), ('start', 237), ('rwait', (155, 161, 291)),
     ('recv', 161, 1), ('prep', 238, 1), ('start', 238), ('rwait', (295,)), ('prep', 239, 2),
     ('prep', 240, 2), ('start', 239), ('start', 240), ('rwait', (297, 164)), ('prep', 241, 1),
     ('start', 241), ('wait', (('wo',),)), ('recv', 284, 1), ('recv', 291, 1), ('prep', 242, 1),
     ('start', 242), ('fence',), ('wocast',), ('rwait', (163,)), ('prep', 243, 0), ('start', 243),
     ('rwait', (299,)), ('prep', 244, 2), ('recv', 163, 3), ('prep', 245, 3), ('start', 244),
     ('start', 245), ('rwait', (300, 159)), ('recv', 159, 2), ('prep', 246, 2), ('recv', 155, 0),
     ('prep', 247, 0), ('start', 246), ('start', 247), ('rwait', (301,)), ('recv', 301, 1),
     ('prep', 248, 1), ('start', 248), ('rwait', (304, 305)), ('recv', 304, 2), ('prep', 249, 2),
     ('start', 249), ('rwait', (306,)), ('recv', 164, 2), ('prep', 250, 2), ('recv', 300, 0),
     ('prep', 251, 0), ('prep', 252, 3), ('start', 250), ('start', 251), ('start', 252),
     ('rwait', (308,)), ('recv', 308, 3), ('prep', 253, 3), ('prep', 254, 0), ('start', 253),
     ('start', 254), ('rwait', (165,)), ('recv', 165, 3), ('prep', 255, 3), ('start', 255),
     ('rwait', (310, 314)), ('prep', 256, 1), ('start', 256), ('rwait', (319,)), ('prep', 257, 3),
     ('start', 257), ('rwait', (168, 317)), ('recv', 310, 2), ('recv', 317, 2), ('prep', 258, 2),
     ('start', 258), ('rwait', (177, 171, 186, 174)), ('ctx', 1, 1), ('rwait', (323, 189)),
     ('out', 1, 1), ('recv', 305, 0), ('recv', 314, 1), ('recv', 319, 3), ('ctx', 0, 2),
     ('rwait',
      (191, 181, 324, 183, 187, 184, 192, 321, 326, 332, 330, 331, 190, 329, 327, 185, 188, 328)),
     ('recv', 327, 0), ('recv', 332, 1), ('recv', 187, 2), ('recv', 189, 3), ('recv', 181, 0),
     ('recv', 183, 1), ('recv', 185, 2), ('recv', 191, 3), ('ctx', 0, 3), ('out', 0, 2),
     ('recv', 186, 1), ('ctx', 1, 2), ('recv', 321, 0), ('recv', 329, 1), ('recv', 330, 2),
     ('recv', 328, 3), ('recv', 323, 0), ('recv', 331, 1), ('recv', 326, 2), ('recv', 324, 3),
     ('ctx', 1, 0), ('out', 1, 2), ('rwait', (194, 333, 175, 334, 193, 336, 173, 335)),
     ('out', 1, 0), ('recv', 297, 0), ('recv', 295, 1), ('recv', 299, 2), ('recv', 306, 3),
     ('recv', 333, 0), ('recv', 334, 1), ('recv', 335, 2), ('recv', 171, 3), ('recv', 282, 3),
     ('ctx', 1, 3), ('recv', 193, 0), ('recv', 336, 1), ('recv', 194, 2), ('recv', 188, 3),
     ('recv', 175, 0), ('recv', 184, 1), ('recv', 192, 2), ('recv', 190, 3), ('ctx', 0, 0),
     ('out', 0, 3), ('recv', 173, 0), ('recv', 168, 1), ('recv', 174, 2), ('recv', 177, 3),
     ('ctx', 0, 1), ('out', 0, 0), ('out', 1, 3), ('out', 0, 1)],
 3: [('wait', (('v', 0, 0, 1),)), ('prep', 26, None), ('start', 26), ('wait', (('k', 0, 0, 1),)),
     ('kprep', 0, 0, 1), ('prep', 25, None), ('start', 25), ('wait', (('k', 1, 1, 0),)),
     ('prep', 28, None), ('start', 28), ('wait', (('v', 0, 0, 0), ('k', 0, 1, 1))),
     ('kprep', 1, 1, 0), ('kprep', 0, 1, 1), ('bar',), ('prep', 31, None), ('start', 31),
     ('wait', (('k', 1, 1, 1),)), ('prep', 29, None), ('start', 29), ('wait', (('k', 0, 1, 0),)),
     ('prep', 33, None), ('kprep', 1, 1, 1), ('start', 33),
     ('wait', (('x', 1, 1), ('v', 0, 1, 1), ('wq', 1))), ('prep', 32, None), ('prep', 30, None),
     ('q', 1, 1, 1), ('start', 32), ('start', 30), ('wait', (('k', 0, 0, 0),)), ('s', 1, 1, 1),
     ('kprep', 0, 0, 0), ('kprep', 0, 1, 0), ('wait', (('x', 0, 0), ('v', 1, 1, 1))),
     ('rwait', (4,)), ('pv', 1, 1, 1), ('prep', 259, 0), ('prep', 27, None), ('q', 0, 0, 1),
     ('prep', 260, 2), ('prep', 261, 3), ('recv', 4, None), ('s', 0, 2, 0), ('s', 0, 0, 1),
     ('start', 259), ('start', 27), ('start', 260), ('start', 261), ('rwait', (6,)),
     ('wait', (('v', 1, 1, 0),)), ('prep', 262, 1), ('start', 262), ('wait', (('v', 0, 1, 0),)),
     ('prep', 34, None), ('pv', 0, 0, 1), ('prep', 263, 0), ('recv', 6, None), ('s', 0, 3, 1),
     ('pv', 0, 2, 0), ('prep', 264, 1), ('start', 34), ('start', 263), ('start', 264),
     ('wait', (('x', 1, 0), ('x', 1, 3))), ('pv', 0, 3, 1), ('q', 1, 0, 1), ('prep', 265, 0),
     ('start', 265), ('rwait', (5, 19)), ('prep', 266, 1), ('start', 266), ('rwait', (35,)),
     ('prep', 267, 3), ('prep', 268, 2), ('recv', 35, 0), ('prep', 269, 0), ('start', 267),
     ('start', 268), ('start', 269), ('rwait', (36,)), ('wait', (('k', 1, 0, 1),)),
     ('prep', 270, 3), ('recv', 19, None), ('s', 1, 0, 1), ('q', 1, 3, 1), ('start', 270),
     ('rwait', (37,)), ('recv', 37, 3), ('prep', 271, 3), ('prep', 272, 2), ('start', 271),
     ('start', 272), ('wait', (('wq', 0), ('k', 1, 0, 0))), ('rwait', (38, 20)), ('recv', 20, None),
     ('pv', 1, 0, 1), ('recv', 38, 2), ('prep', 273, 2), ('prep', 274, 0), ('s', 1, 3, 1),
     ('q', 1, 3, 0), ('q', 1, 0, 0), ('recv', 36, 1), ('prep', 275, 1), ('prep', 276, 3),
     ('kprep', 1, 0, 1), ('kprep', 1, 0, 0), ('prep', 277, 2), ('q', 1, 1, 0), ('start', 273),
     ('start', 274), ('start', 275), ('start', 276), ('start', 277), ('rwait', (21,)),
     ('prep', 278, 1), ('start', 278), ('rwait', (42, 40)),
     ('wait', (('x', 1, 2), ('v', 1, 0, 0), ('v', 1, 0, 1))), ('recv', 42, 0), ('prep', 279, 0),
     ('pv', 1, 3, 1), ('recv', 21, None), ('s', 1, 0, 0), ('s', 1, 3, 0), ('q', 1, 2, 0),
     ('prep', 280, 3), ('s', 1, 1, 0), ('prep', 281, 0), ('start', 279), ('start', 280),
     ('start', 281), ('rwait', (45,)), ('prep', 282, 3), ('prep', 283, 2), ('start', 282),
     ('start', 283), ('rwait', (22, 41)), ('recv', 41, 1), ('prep', 284, 1), ('prep', 285, 1),
     ('start', 284), ('start', 285), ('fence',), ('recv', 22, None), ('pv', 1, 0, 0),
     ('prep', 286, 3), ('pv', 1, 1, 0), ('prep', 287, 0), ('pv', 1, 3, 0), ('recv', 40, 2),
     ('prep', 288, 2), ('prep', 289, 1), ('recv', 45, 3), ('prep', 290, 3), ('prep', 291, 1),
     ('prep', 292, 0), ('start', 286), ('start', 287), ('start', 288), ('start', 289),
     ('start', 290), ('start', 291), ('start', 292), ('rwait', (52,)), ('s', 1, 2, 0),
     ('rwait', (23, 53, 57)), ('prep', 293, 2), ('recv', 52, 0), ('prep', 294, 0), ('recv', 53, 1),
     ('prep', 295, 1), ('start', 293), ('start', 294), ('start', 295), ('rwait', (39, 58)),
     ('recv', 57, 3), ('prep', 296, 3), ('start', 296), ('rwait', (43,)), ('pv', 1, 2, 0),
     ('prep', 297, 0), ('recv', 58, 2), ('prep', 298, 2), ('prep', 299, 2), ('recv', 39, 0),
     ('prep', 300, 0), ('recv', 43, 1), ('prep', 301, 1), ('recv', 5, None), ('recv', 23, None),
     ('s', 0, 2, 1), ('prep', 302, 1), ('start', 297), ('start', 298), ('start', 299),
     ('start', 300), ('start', 301), ('start', 302), ('rwait', (60, 24)), ('recv', 24, None),
     ('pv', 0, 2, 1), ('rwait', (61, 140)), ('recv', 140, 0), ('prep', 303, 0), ('start', 303),
     ('rwait', (66,)), ('recv', 60, 2), ('prep', 304, 2), ('recv', 66, 0), ('prep', 305, 0),
     ('start', 304), ('start', 305), ('rwait', (141,)), ('prep', 306, 3), ('start', 306),
     ('rwait', (142, 68)), ('recv', 141, 2), ('prep', 307, 2), ('start', 307), ('rwait', (143, 69)),
     ('recv', 61, 3), ('prep', 308, 3), ('recv', 143, 3), ('prep', 309, 3), ('start', 308),
     ('start', 309), ('fence',), ('prep', 310, 2), ('start', 310), ('rwait', (71,)),
     ('recv', 142, 1), ('prep', 311, 1), ('start', 311), ('rwait', (204,)), ('recv', 204, 0),
     ('prep', 312, 0), ('start', 312), ('rwait', (205, 70)), ('recv', 205, 1), ('prep', 313, 1),
     ('start', 313), ('rwait', (206, 74)), ('recv', 70, 1), ('prep', 314, 1), ('recv', 206, 3),
     ('prep', 315, 3), ('start', 314), ('start', 315), ('rwait', (209,)), ('wait', (('wo',),)),
     ('recv', 209, 2), ('prep', 316, 2), ('start', 316), ('rwait', (72,)), ('recv', 69, 2),
     ('prep', 317, 2), ('start', 317), ('rwait', (212,)), ('recv', 212, 0), ('prep', 318, 0),
     ('recv', 68, 3), ('prep', 319, 3), ('start', 318), ('start', 319), ('rwait', (213, 78, 80)),
     ('recv', 213, 1), ('prep', 320, 1), ('recv', 80, 0), ('prep', 321, 0), ('start', 320),
     ('start', 321), ('rwait', (214, 76)), ('recv', 214, 2), ('prep', 322, 2), ('recv', 71, 0),
     ('prep', 323, 0), ('start', 322), ('start', 323), ('rwait', (77,)), ('recv', 72, 3),
     ('prep', 324, 3), ('start', 324), ('rwait', (215,)), ('recv', 215, 3), ('prep', 325, 3),
     ('start', 325), ('rwait', (82, 87)), ('recv', 82, 2), ('prep', 326, 2), ('prep', 327, 0),
     ('recv', 77, 3), ('prep', 328, 3), ('start', 326), ('start', 327), ('start', 328),
     ('rwait', (225, 85)), ('recv', 85, 1), ('prep', 329, 1), ('start', 329), ('rwait', (93, 99)),
     ('recv', 76, 2), ('prep', 330, 2), ('recv', 78, 1), ('ctx', 1, 0), ('start', 330),
     ('rwait', (233, 101, 104, 222)), ('prep', 331, 1), ('start', 331), ('rwait', (97, 235, 108)),
     ('prep', 332, 1), ('start', 332), ('fence',), ('prep', 333, 0), ('start', 333),
     ('rwait', (95, 92, 106, 111, 231, 103, 113)), ('recv', 74, 1), ('prep', 334, 1),
     ('start', 334), ('fence',), ('wocast',), ('rwait', (228, 229)), ('prep', 335, 2),
     ('start', 335), ('rwait', (116, 220, 90, 114)), ('prep', 336, 1), ('start', 336),
     ('rwait', (240, 169, 238, 172)), ('out', 1, 0), ('rwait', (118, 250, 119)), ('recv', 101, 0),
     ('recv', 108, 2), ('recv', 119, 3), ('ctx', 1, 3), ('recv', 87, 0), ('recv', 104, 1),
     ('recv', 90, 2), ('recv', 93, 3), ('recv', 95, 0), ('recv', 97, 1), ('recv', 99, 2),
     ('recv', 114, 3), ('ctx', 0, 3), ('recv', 220, 0), ('recv', 222, 1), ('recv', 225, 2),
     ('recv', 233, 3), ('ctx', 1, 1), ('recv', 231, 0), ('recv', 229, 1), ('recv', 240, 2),
     ('recv', 228, 3), ('ctx', 0, 2), ('out', 0, 3), ('out', 1, 3),
     ('rwait', (123, 130, 179, 124, 247, 255, 246, 245)), ('out', 1, 1), ('out', 0, 2),
     ('recv', 111, 0), ('recv', 116, 1), ('recv', 118, 2), ('recv', 92, 3), ('recv', 106, 0),
     ('recv', 103, 1), ('recv', 113, 2), ('recv', 123, 3), ('ctx', 0, 0), ('recv', 235, 0),
     ('recv', 238, 1), ('recv', 246, 2), ('recv', 255, 3), ('recv', 124, 0), ('recv', 172, 1),
     ('recv', 169, 2), ('recv', 130, 3), ('ctx', 0, 1), ('recv', 247, 0), ('recv', 179, 1),
     ('recv', 250, 2), ('recv', 245, 3), ('ctx', 1, 2), ('out', 1, 2), ('out', 0, 0),
     ('out', 0, 1)]}

_KERNEL = build(dict(
    msgs=[dict(src=s, dst=d, b=b, q=q, p=p, subs=h, set=z if isinstance(z, str) else frozenset(z))
          for s, d, b, q, p, h, z in _MSGS],
    loads=_LOADS, prog=_PROG))


def pallas_dist_sparse_attn_blocksparse_kvseq_b2_sq256_skv256_hq4_dh64_kernel(x, Wq, K_ext, V_ext, Wo):
    return _KERNEL(x, Wq, K_ext, V_ext, Wo)
```
